```python
import numpy as np

kernel_name = "dist_max_ax1_xy_m2048_n1024"

def setup_inputs():
    return {"x": np.random.randn(4096, 2048).astype(np.float32)}

def reference(x: np.ndarray) -> np.ndarray:
    return np.max(x, axis=1, keepdims=True)
```

```python
import jax
import jax.numpy as jnp
from jax import lax
from jax.experimental import pallas as pl
from jax.experimental.pallas import tpu as pltpu

M, N = 2048, 1024
LANES = 128
NB = M // LANES
HB = NB // 2
NEG = float("-inf")
MESH = pl.DeviceIdType.MESH

CHUNKS1 = (512, 512)
CHUNKS2 = (512, 256, 128)
TAIL = ((80, True), (40, False), (8, True))
S_ROWS = 48

_SIZES = list(CHUNKS1) + list(CHUNKS2) + [t[0] for t in TAIL]
_OFFS = [sum(_SIZES[:i]) for i in range(len(_SIZES))]
_NC = len(_SIZES)
_XC = len(CHUNKS1) + len(CHUNKS2) - 1


def _body(x_hbm, out_ref, xbuf, psend, precv, sbuf):
    mx = lax.axis_index("x")
    my = lax.axis_index("y")
    nbr = (mx, 1 - my)
    half = M // 2
    base1 = pl.multiple_of((1 - my) * half, half)
    base2 = pl.multiple_of(my * half, half)
    ob = my * HB
    oo = (1 - my) * HB

    def colmax(r0, rows):
        v = [xbuf[pl.ds(r0, rows), j * LANES:(j + 1) * LANES]
             for j in range(N // LANES)]
        while len(v) > 1:
            v = [jnp.maximum(v[i], v[i + 1]) for i in range(0, len(v), 2)]
        return v[0]

    def diag(m, off):
        rows = m.shape[0]
        r = jnp.max(m, axis=1, keepdims=True)
        row = lax.broadcasted_iota(jnp.int32, (rows, LANES), 0)
        col = lax.broadcasted_iota(jnp.int32, (rows, LANES), 1)
        return jnp.where(col == row + off,
                         jnp.broadcast_to(r, (rows, LANES)), NEG)

    def rowmax(r0):
        return jnp.max(diag(colmax(r0, LANES), 0), axis=0, keepdims=True)

    def main(in_sems, send_sems, recv1, smem_sem, recv2):
        copies = []
        h2s = None
        for c in range(_NC):
            o, s = _OFFS[c], _SIZES[c]
            if c == _XC:
                o, s = o + S_ROWS, s - S_ROWS
            src = base1 + o if o < half else base2 + (o - half)
            cp = pltpu.make_async_copy(
                x_hbm.at[pl.ds(src, s), :], xbuf.at[pl.ds(o, s), :],
                in_sems.at[c])
            cp.start()
            copies.append(cp)
            if c == 0:
                h2s = pltpu.make_async_copy(
                    x_hbm.at[pl.ds(base2 + (_OFFS[_XC] - half), S_ROWS), :],
                    sbuf, smem_sem)
                h2s.start()
        barrier = pltpu.get_barrier_semaphore()
        pl.semaphore_signal(barrier, inc=1, device_id=nbr, device_id_type=MESH)
        s2v = pltpu.make_async_copy(
            sbuf, xbuf.at[pl.ds(_OFFS[_XC], S_ROWS), :], smem_sem)

        c = 0
        for s in CHUNKS1:
            copies[c].wait()
            b0 = _OFFS[c] // LANES
            for b in range(b0, b0 + s // LANES):
                psend[b] = rowmax(b * LANES)
            if c == 0:
                h2s.wait()
                s2v.start()
            c += 1
        pl.semaphore_wait(barrier, 1)
        rd1 = pltpu.make_async_remote_copy(
            psend, precv, send_sems.at[0], recv1,
            device_id=nbr, device_id_type=MESH)
        rd1.start()

        for k, s in enumerate(CHUNKS2):
            copies[c].wait()
            if k == 0:
                rd1.wait_recv()
            if c == _XC:
                s2v.wait()
            b0 = _OFFS[c] // LANES - HB
            for b in range(b0, b0 + s // LANES):
                out_ref[ob + b] = jnp.maximum(
                    rowmax((HB + b) * LANES), precv[b])
            c += 1
        rows2 = out_ref.at[pl.ds(ob, HB - 1)]
        rd2 = pltpu.make_async_remote_copy(
            rows2, rows2, send_sems.at[1], recv2,
            device_id=nbr, device_id_type=MESH)
        rd2.start()

        acc = jnp.broadcast_to(precv[HB - 1], (8, LANES))
        off = 0
        pending = []
        for s, reduce_now in TAIL:
            copies[c].wait()
            pending.append((colmax(_OFFS[c], s), off))
            if reduce_now:
                for m, o in pending:
                    d = diag(m, o)
                    for g in range(m.shape[0] // 8):
                        acc = jnp.maximum(acc, d[g * 8:(g + 1) * 8])
                pending = []
            off += s
            c += 1
        out_ref[ob + HB - 1] = jnp.max(acc, axis=0, keepdims=True)
        rows3 = out_ref.at[pl.ds(ob + HB - 1, 1)]
        rd3 = pltpu.make_async_remote_copy(
            rows3, rows3, send_sems.at[2], recv2,
            device_id=nbr, device_id_type=MESH)
        rd3.start()

        rd1.wait_send()
        rd2.wait_send()
        rd3.wait_send()
        theirs = out_ref.at[pl.ds(oo, HB)]
        pltpu.make_async_copy(theirs, theirs, recv2).wait()

    pl.run_scoped(
        main,
        pltpu.SemaphoreType.DMA((_NC,)),
        pltpu.SemaphoreType.DMA((3,)),
        pltpu.SemaphoreType.DMA,
        pltpu.SemaphoreType.DMA,
        pltpu.SemaphoreType.DMA,
    )


def pallas_dist_max_ax1_xy_m2048_n1024_kernel(x: jax.Array):
    out = pl.pallas_call(
        _body,
        out_shape=jax.ShapeDtypeStruct((NB, 1, LANES), jnp.float32),
        in_specs=[pl.BlockSpec(memory_space=pl.ANY)],
        out_specs=pl.BlockSpec(memory_space=pltpu.VMEM),
        scratch_shapes=[
            pltpu.VMEM((M, N), jnp.float32),
            pltpu.VMEM((HB, 1, LANES), jnp.float32),
            pltpu.VMEM((HB, 1, LANES), jnp.float32),
            pltpu.SMEM((S_ROWS, N), jnp.float32),
        ],
        compiler_params=pltpu.CompilerParams(collective_id=0),
    )(x)
    return out.reshape(M, 1)
```

```python
import jax
import jax.numpy as jnp
from jax import lax
from jax.experimental import pallas as pl
from jax.experimental.pallas import tpu as pltpu

M, N = 2048, 1024
L = 128
NB = M // L
HB = NB // 2
H = M // 2
NEG = float("-inf")
MESH = pl.DeviceIdType.MESH

P1, P2 = 64, 40
P = P1 + P2
X = 80
S_ROWS = (48, 56)
S_OFF = H + 4 * L
FIRST = (512, 512)
SECOND = ((512, 256, 128, 80, 40, 8),
          (512, 320, 64, 40, 8))
N_CHUNKS = len(FIRST) + max(len(s) for s in SECOND)


def _colmax(buf, r0, rows):
    v = [buf[pl.ds(r0, rows), j * L:(j + 1) * L] for j in range(N // L)]
    while len(v) > 1:
        v = [jnp.maximum(v[i], v[i + 1]) for i in range(0, len(v), 2)]
    return v[0]


def _diag(m, off):
    rows = m.shape[0]
    r = jnp.max(m, axis=1, keepdims=True)
    row = lax.broadcasted_iota(jnp.int32, (rows, L), 0)
    col = lax.broadcasted_iota(jnp.int32, (rows, L), 1)
    return jnp.where(col == row + off, jnp.broadcast_to(r, (rows, L)), NEG)


def _fold(acc, d):
    for g in range(d.shape[0] // 8):
        acc = jnp.maximum(acc, d[g * 8:(g + 1) * 8])
    return acc


def _rowmax(buf, r0, rows):
    return jnp.max(_diag(_colmax(buf, r0, rows), 0), axis=0, keepdims=True)


def _program(my, mx, x_hbm, out_ref, xbuf, psend, precv, sbuf, rbuf, qsend,
             qrecv, in_sems, send_sems, smem_sem, recv_p, recv_out, recv_raw,
             recv_q):
    late = my == 1
    ynbr = (mx, 1 - my)
    xnbr = (1 - mx, my)
    s_rows = S_ROWS[my]
    p_out = P if late else 0
    x_out = X if late else 0
    ob = my * HB

    def src_row(o):
        return (1 - my) * H + o if o < H else my * H + (o - H)

    spans = []
    o = 0
    for s in FIRST + SECOND[my]:
        if o == M - L:
            o += x_out
        spans.append((o, s))
        o += s
    assert o == M

    copies = []
    h2s = pltpu.make_async_copy(
        x_hbm.at[pl.ds(src_row(S_OFF), s_rows), :],
        sbuf.at[pl.ds(0, s_rows), :], smem_sem)
    for c, (o, s) in enumerate(spans):
        if o + s == H:
            s -= p_out
        if o == S_OFF:
            o, s = o + s_rows, s - s_rows
        cp = pltpu.make_async_copy(
            x_hbm.at[pl.ds(src_row(o), s), :], xbuf.at[pl.ds(o, s), :],
            in_sems.at[c])
        cp.start()
        copies.append(cp)
        if c == 0:
            h2s.start()
    s2v = pltpu.make_async_copy(
        sbuf.at[pl.ds(0, s_rows), :], xbuf.at[pl.ds(S_OFF, s_rows), :],
        smem_sem)

    barrier = pltpu.get_barrier_semaphore()
    pl.semaphore_signal(barrier, inc=1, device_id=ynbr, device_id_type=MESH)
    if late:
        pl.semaphore_signal(barrier, inc=1, device_id=xnbr,
                            device_id_type=MESH)
    pl.semaphore_wait(barrier, 2 if late else 1)

    sends = []

    def rdma(src, dst, recv_sem, device):
        rd = pltpu.make_async_remote_copy(
            src, dst, send_sems.at[len(sends)], recv_sem,
            device_id=device, device_id_type=MESH)
        rd.start()
        sends.append(rd)
        return rd

    def push_y(p0, rows):
        rdma(x_hbm.at[pl.ds(src_row(H - P + p0), rows), :],
             rbuf.at[pl.ds(p0, rows), :], recv_raw, ynbr)

    if late:
        push_y(0, P1)
        raw_x = rdma(x_hbm.at[pl.ds(src_row(M - L), X), :],
                     rbuf.at[pl.ds(0, X), :], recv_raw, xnbr)

    for c in range(len(FIRST)):
        o, s = spans[c]
        copies[c].wait()
        for b in range(o // L, (o + s) // L):
            psend[b] = _rowmax(xbuf, b * L, L - (p_out if b == HB - 1 else 0))
        if c == 0:
            h2s.wait()
            s2v.start()
    part = rdma(psend, precv, recv_p, ynbr)
    if late:
        push_y(P1, P2)
        raw_x.wait_recv()
        qsend[...] = _rowmax(rbuf, 0, X)
        q = rdma(qsend, qrecv, recv_q, xnbr)

    acc = {}
    pending = []
    for c in range(len(FIRST), len(spans)):
        o, s = spans[c]
        copies[c].wait()
        if o == H:
            part.wait_recv()
        if o == S_OFF:
            s2v.wait()
        r = o
        while r < o + s:
            e = min(o + s, (r // L + 1) * L)
            pending.append((_colmax(xbuf, r, e - r), r))
            r = e
        if c != len(spans) - 2:
            for m, r in pending:
                b = r // L - HB
                if b not in acc:
                    acc[b] = jnp.broadcast_to(precv[b], (8, L))
                acc[b] = _fold(acc[b], _diag(m, r % L))
                if (r + m.shape[0]) % L == 0 and b < HB - 1:
                    out_ref[ob + b] = jnp.max(acc[b], axis=0, keepdims=True)
            pending = []
        if o + s == M - L:
            rows = out_ref.at[pl.ds(ob, HB - 1)]
            rdma(rows, rows, recv_out, ynbr)
            if late:
                q.wait_recv()
                acc[HB - 1] = jnp.broadcast_to(
                    jnp.maximum(precv[HB - 1], qrecv[...]), (8, L))
    last = acc[HB - 1]
    if not late:
        raw = rbuf.at[pl.ds(0, P), :]
        pltpu.make_async_copy(raw, raw, recv_raw).wait()
        last = _fold(last, _diag(_colmax(rbuf, 0, P), L - P))
    out_ref[ob + HB - 1] = jnp.max(last, axis=0, keepdims=True)
    rows = out_ref.at[pl.ds(ob + HB - 1, 1)]
    rdma(rows, rows, recv_out, ynbr)

    for rd in sends:
        rd.wait_send()
    theirs = out_ref.at[pl.ds((1 - my) * HB, HB)]
    pltpu.make_async_copy(theirs, theirs, recv_out).wait()


def _body(*refs):
    mx = lax.axis_index("x")
    my = lax.axis_index("y")

    def scoped(*sems):
        @pl.when(my == 1)
        def _():
            _program(1, mx, *refs, *sems)

        @pl.when(my == 0)
        def _():
            _program(0, mx, *refs, *sems)

    dma = pltpu.SemaphoreType.DMA
    pl.run_scoped(scoped, dma((N_CHUNKS,)), dma((7,)), dma, dma, dma, dma, dma)


def pallas_dist_max_ax1_xy_m2048_n1024_kernel(x: jax.Array):
    out = pl.pallas_call(
        _body,
        out_shape=jax.ShapeDtypeStruct((NB, 1, L), jnp.float32),
        in_specs=[pl.BlockSpec(memory_space=pl.ANY)],
        out_specs=pl.BlockSpec(memory_space=pltpu.VMEM),
        scratch_shapes=[
            pltpu.VMEM((M, N), jnp.float32),
            pltpu.VMEM((HB, 1, L), jnp.float32),
            pltpu.VMEM((HB, 1, L), jnp.float32),
            pltpu.SMEM((max(S_ROWS), N), jnp.float32),
            pltpu.VMEM((max(P, X), N), jnp.float32),
            pltpu.VMEM((1, L), jnp.float32),
            pltpu.VMEM((1, L), jnp.float32),
        ],
        compiler_params=pltpu.CompilerParams(collective_id=0),
    )(x)
    return out.reshape(M, 1)
```
